```python
import numpy as np

kernel_name = "dist_sparse_attn_localglobal_htp_kvseq_b2_sq256_skv256_hq4_dh64"

def setup_inputs():
    x = np.random.randn(2, 256, 512).astype(np.float32)
    Wq = np.random.randn(512, 1024).astype(np.float32) * 0.02
    K_ext = np.random.randn(2, 1024, 16, 64).astype(np.float32)
    V_ext = np.random.randn(2, 1024, 16, 64).astype(np.float32)
    Wo = np.random.randn(1024, 512).astype(np.float32) * 0.02
    return {"x": x, "Wq": Wq, "K_ext": K_ext, "V_ext": V_ext, "Wo": Wo}

def reference(x, Wq, K_ext, V_ext, Wo):
    B, Sq, Skv, Hq, Dh = 2, 256, 1024, 16, 64
    Q = (x @ Wq).reshape(B, Sq, Hq, Dh)
    qi = np.arange(Sq)[:, None]
    ki = np.arange(Skv)[None, :]
    local = np.abs(qi - ki) <= 128
    glob = (ki < 32) | (qi < 32)
    mask = local | glob
    scores = np.einsum('bihd,bjhd->bhij', Q, K_ext).astype(np.float32) * 0.125
    scores = np.where(mask[None, None, :, :], scores, -1e9)
    scores_max = scores.max(axis=-1, keepdims=True)
    w = np.exp(scores - scores_max)
    row_keep = mask.any(axis=1)
    w_sum = np.where(row_keep[None, None, :, None], w.sum(axis=-1, keepdims=True), 1.0)
    w = w / w_sum
    w = np.where(row_keep[None, None, :, None], w, 0.0)
    ctx = np.einsum('bhij,bjhd->bihd', w, V_ext).reshape(B, Sq, Hq * Dh)
    return ctx @ Wo
```

```python
import functools

import jax
import jax.numpy as jnp
from jax import lax
from jax.experimental import pallas as pl
from jax.experimental.pallas import tpu as pltpu

F32 = jnp.float32
BF16 = jnp.bfloat16
MESH = pl.DeviceIdType.MESH
NEG = -1e9
QSCALE = 0.125 * 1.4426950408889634
NT = (((1,), (1,)), ((), ()))
PAIR = {"": pl.ds(0, 256), "a": pl.ds(0, 128), "b": pl.ds(128, 128)}
A_PIECE = {"": (0, 256), "a": (0, 32), "b": (32, 96), "v": (128, 128)}


def _dot(a, b):
    return jnp.dot(a, b, preferred_element_type=F32)


def _dot_nt(a, b):
    return lax.dot_general(a, b, NT, preferred_element_type=F32)


def _iota(shape, d):
    return lax.broadcasted_iota(jnp.int32, shape, d)


def _blockdiag(w):
    top = _iota(w.shape, 0) < 64
    z = jnp.zeros_like(w)
    return jnp.concatenate([jnp.where(top, w, z), jnp.where(top, z, w)], axis=1)


def _masks(half):
    qi = _iota((128, 128), 0)
    ki = _iota((128, 128), 1)
    if half == 0:
        return [None, (qi < 32) | (ki <= qi)]
    return [(ki < 32) | (ki >= qi), None, ki <= qi]


def _scores(q2, kt, masks):
    s = _dot(q2, _blockdiag(kt))
    nt = len(masks)
    tile = lambda i: s[:, 128 * i:128 * i + 128]
    return [[tile(h * nt + t) if m is None else jnp.where(m, tile(h * nt + t), NEG)
             for t, m in enumerate(masks)] for h in range(2)]


def _softmax(heads):
    ps, st = [], []
    for ts in heads:
        m = jnp.max(functools.reduce(jnp.maximum, ts), axis=1, keepdims=True)
        e = [jnp.exp2(x - m) for x in ts]
        st.append((m, jnp.sum(functools.reduce(jnp.add, e), axis=1, keepdims=True)))
        ps += [x.astype(BF16) for x in e]
    lo = _iota((ps[0].shape[0], 128), 1) < 64
    return jnp.concatenate(ps, axis=1), jnp.where(lo, 1.0 / st[0][1], 1.0 / st[1][1]), st


def _lse(stats, rows):
    return [m[:rows] + jnp.log2(l[:rows]) for m, l in stats]


def _pack(cols, width, head0):
    n = 128 // width
    lane = _iota((n, 128), 1) - width * _iota((n, 128), 0)
    out = []
    for r0 in range(0, cols[0].shape[0], n):
        v = functools.reduce(jnp.add, [jnp.where(lane == head0 + i, c[r0:r0 + n], 0.0)
                                       for i, c in enumerate(cols)])
        out.append(jnp.sum(v, axis=0, keepdims=True))
    return jnp.concatenate(out, axis=0)


def _merge(terms, width):
    n = 128 // width
    r = terms[0][0].shape[0]
    m = functools.reduce(jnp.maximum, [t[1] for t in terms])
    ws = [jnp.exp2(t[1] - m) for t in terms]
    tot = functools.reduce(jnp.add, ws)
    inv = 1.0 / tot
    own = _iota((n, 128), 1) // width == _iota((n, 128), 0)
    lhs = [jnp.where(own, (w * inv)[j:j + 1], 0.0) for w in ws for j in range(r // n)]
    spread = _iota((128, 64 * width), 0) % width == _iota((128, 64 * width), 1) // 64
    e = _dot(jnp.concatenate(lhs, axis=0).astype(BF16), jnp.where(spread, 1.0, 0.0).astype(BF16))
    ctx = functools.reduce(jnp.add, [e[r * k:r * k + r] * t[0] for k, t in enumerate(terms)])
    return ctx, m + jnp.log2(tot)


def _build(plan, trees, **debug):
    def number(kind, keep):
        idx, most = {}, 1
        for c in range(4):
            names = [op[2:] for op in plan[c] if op[0] == kind and keep(op[2:])]
            idx.update({(c, n) if kind == "L" else n: i for i, n in enumerate(names)})
            most = max(most, len(names))
        return idx, most

    with_lse = lambda n: n[0] == "C" or (n[0] == "Z" and n[-1] == "b")
    lsem_of, n_l = number("L", lambda n: True)
    ssem_of, n_s = number("S", lambda n: True)
    rsem_of, n_r = number("W", lambda n: n in ssem_of)
    s2_of, n_s2 = number("S", with_lse)
    r2_of, n_r2 = number("W", with_lse)
    gs_of, n_gs = number("S", lambda n: n[0] == "C")
    gr_of, n_gr = number("W", lambda n: n[0] == "C")
    sb_of, n_sb = number("S", lambda n: n[0] == "R")
    rb_of, n_rb = number("W", lambda n: n[0] == "R")
    nlead = {c: next(i for i, op in enumerate(plan[c]) if op[0] != "L") for c in range(4)}

    as_ctx = lambda s, d, sites: (s, d, sites) == (2, 1, "2")
    r_src, staged = {}, set()
    for piece, steps in trees.items():
        have = {}
        for s, d, sites in steps:
            n = f"R{piece}_{s}{d}{sites}"
            if not as_ctx(s, d, sites):
                if (s, sites) not in have:
                    have[s, sites] = ("s", n)
                    staged.add(n)
                r_src[n] = have[s, sites]
                have.setdefault((d, sites), ("r", n))

    def body(x_hbm, wq_hbm, kt_hbm, vt_hbm, wo_hbm, out_ref,
             xf, wqf, wof, kf, vf, wqb, wob, kvs, kvr, a1s, a1r, qa, qb, qg,
             gctx, gl, l0, gs_c, gs_l, gr_c, gr_l, ctxa, ctxb, pbuf, ibuf,
             yq, yc, yl_s, yl_r, ubuf, wbuf, sb, rb, tick, park,
             lsem, ssem, rsem, ssem2, rsem2, rdy):
        me = lax.axis_index("i")

        def hrows(g, p):
            return pl.ds(256 * g + 128 * p, 128)

        def prow(blk):
            return pl.ds(256 * int(blk[0]) + 16 * int(blk[1], 16), 16)

        def orows(blk):
            return out_ref.at[int(blk[0]), pl.ds(16 * int(blk[1], 16), 16)]

        def slot(kind, n):
            return sb.at[sb_of[n]] if kind == "s" else rb.at[rb_of[n]]

        def load(c, n):
            sem = lsem.at[lsem_of[c, n]]
            if n == "xg":
                src, dst = x_hbm.at[:, pl.ds(0, 32)], xf.at[:, pl.ds(0, 32)]
            elif n[0] == "x":
                src, dst = x_hbm.at[int(n[2]), pl.ds(32, 224)], xf.at[int(n[2]), pl.ds(32, 224)]
            elif n[:2] == "wq":
                src, dst = wq_hbm.at[:, PAIR[n[2:]]], wqf.at[:, PAIR[n[2:]]]
            elif n[0] == "w":
                r = pl.ds(16 * int(n[2], 36), 16 * int(n[3], 36))
                src, dst = wo_hbm.at[r], wof.at[r]
            else:
                src, dst = (kt_hbm, kf) if n[0] == "k" else (vt_hbm, vf)
                r0, nr = A_PIECE[n[4:]] if n[4:] in ("a", "b") else (0, 128 * int(n[3]))
                at = (slice(None) if n[1] == "2" else int(n[1]), pl.ds(128 * int(n[2]) + r0, nr),
                      {"": pl.ds(0, 256), "h": pl.ds(128, 128)}.get(n[4:], pl.ds(0, 128)))
                src, dst = src.at[at], dst.at[at]
            return pltpu.make_async_copy(src, dst, sem)

        def message(n):
            if n[0] in "KV":
                b, g, p, t = int(n[1]), int(n[2]), int(n[3]), "KV".index(n[0])
                via = n[4:5] in ("p", "f")
                r = pl.ds(16 * int(n[5]), 16) if via else pl.ds(*{"": (0, 128), "r": (32, 96)}[n[4:]])
                src, dst = kvs.at[b, g - 1, p, t, r], kvr.at[b, p, t, r]
                if via:
                    return (3, [(src, park.at[r])]) if n[4] == "p" else (2, [(park.at[r], dst)])
                return g, [(src, dst)]
            if n[0] == "A":
                b, g, p, r = int(n[1]), int(n[2]), int(n[3]), pl.ds(*A_PIECE[n[4:]])
                return g % 3, [(a1s.at[b, (0, 0, 2, 1)[g], p, r], a1r.at[b, g // 3, p, r])]
            if n[0] == "W":
                r0, nr = 16 * int(n[3], 36), 16 * int(n[4], 36)
                return int(n[2]), [(wob.at[pl.ds(r0, nr)], wob.at[pl.ds(256 + r0, nr)])]
            if n[:2] == "Qg":
                r = qg.at[int(n[2]), :, PAIR[n[5:]]]
                return int(n[4]), [(r, r)]
            if n[0] == "Q":
                r = pl.ds(256 * int(n[2]) + 128 * int(n[3]), 128)
                return 0, [(qa.at[r], qb.at[r])]
            if n[0] == "C":
                i, j = gs_of[n], gr_of[n]
                return int(n[-1]), [(gs_c.at[i], gr_c.at[j]), (gs_l.at[i], gr_l.at[j])]
            if n[0] == "Y":
                h = int(n[3])
                src = qa.at[pl.ds(256 + 128 * h, 128), pl.ds(128, 128)] if n[1] == "2" else yq.at[h]
                return int(n[2]), [(src, yq.at[h])]
            if n[0] == "Z":
                h, r0 = int(n[2]), 64 * "ab".index(n[3])
                dst = ctxa.at[pl.ds(256 + r0, 64), pl.ds(128, 128)] if h == 0 else yc.at[1, pl.ds(r0, 64)]
                return 2, [(yc.at[h, pl.ds(r0, 64)], dst)] + [(yl_s.at[h], yl_r.at[h])] * (n[3] == "b")
            if n[0] == "T":
                return 3, [(tick.at[0], tick.at[1])]
            if n[0] == "H":
                return 1, [(ctxa.at[prow(n[1:])], ctxb.at[prow(n[1:])])]
            return int(n[6]), [(slot(*r_src[n]), slot("r", n))]

        def copies(n, side=None):
            d, pairs = message(n)
            if side is not None:
                pairs = [(refs[side], refs[side]) for refs in pairs]
            sems = [(ssem.at[ssem_of[n]], rsem.at[rsem_of[n]])]
            if len(pairs) > 1:
                sems.append((ssem2.at[s2_of[n]], rsem2.at[r2_of[n]]))
            return [pltpu.make_async_remote_copy(a, b, ss, rs, device_id=(d,), device_id_type=MESH)
                    for (a, b), (ss, rs) in zip(pairs, sems)]

        def qproj(xv, cols=PAIR[""]):
            return (_dot(xv.astype(BF16), wqb[:, cols]) * QSCALE).astype(BF16)

        def site_kv(c, t, b, g, p, half):
            loc = kf if t == 0 else vf
            w = loc[b, hrows(g, p)].astype(BF16) if c == 0 else kvr[b, p, t]
            if half == 0:
                return w
            if c == 1:
                extra = loc[b, hrows(g, p), pl.ds(0, 128)].astype(BF16)
            else:
                extra = a1r[b, g // 3, p, pl.ds(128 * t, 128)]
            return jnp.concatenate([w, extra], axis=1)

        def compute(c, n, held, got):
            if n[:2] == "cq":
                wqb[:, PAIR[n[2:]]] = wqf[:, PAIR[n[2:]]].astype(BF16)
                if c != 3:
                    l0[...] = jnp.zeros(l0.shape, F32)
                    tick[0] = jnp.zeros(tick.shape[1:], F32)
            elif n[:2] == "cw":
                r = pl.ds(16 * int(n[2], 36), 16 * int(n[3], 36))
                wob[r] = wof[r].astype(BF16)
            elif n[:2] in ("ck", "cv"):
                b, g, p, t = int(n[2]), int(n[3]), int(n[4]), "kv".index(n[1])
                kvs[b, g - 1, p, t] = (kf, vf)[t][b, hrows(g, p)].astype(BF16)
            elif n[:2] == "ca":
                b, g, p = int(n[2]), int(n[3]), int(n[4])
                a = a1s.at[b, (0, 0, 2, 1)[g], p]
                r0, nr = A_PIECE[n[5:]]
                if r0 < 128:
                    nk = min(nr, 128)
                    a[pl.ds(r0, nk)] = kf[b, pl.ds(256 * g + 128 * p + r0, nk), pl.ds(0, 128)].astype(BF16)
                if r0 + nr > 128:
                    a[pl.ds(128, 128)] = vf[b, hrows(g, p), pl.ds(0, 128)].astype(BF16)
            elif n[:2] == "qg":
                xv = jnp.concatenate([xf[0, pl.ds(0, 32)], xf[1, pl.ds(0, 32)]], axis=0)
                qg[c, :, PAIR[n[2:]]] = qproj(xv, PAIR[n[2:]])
            elif n[0] == "q":
                b, r0, nr = int(n[1]), 128 * int(n[2]), 128 * int(n[3])
                qa[pl.ds(256 * b + r0, nr)] = qproj(xf[b, pl.ds(r0, nr)])
            elif n[0] in "aso":
                b, g = int(n[1]), int(n[2])
                jobs = [(int(w[0]), int(w[1])) for w in n[4:].split("_")]
                q_ref, c_ref = (qa, ctxa) if g == c else (qb, ctxb)
                at = lambda p, h: (pl.ds(256 * b + 128 * h, 128), pl.ds(128 * p, 128))
                if n[0] == "o":
                    sm = [(pbuf[h, :, pl.ds(0, 512 + 256 * h)], ibuf[h], None) for p, h in jobs]
                else:
                    sc = [_scores(q_ref[at(p, h)], site_kv(c, 0, b, g, p, h), _masks(h)) for p, h in jobs]
                    sm = [_softmax(x) for x in sc]
                    for (p, h), (_, _, stats) in zip(jobs, sm):
                        if h == 0:
                            l0[g, pl.ds(b, 1)] += _pack(_lse(stats, 32), 4, 2 * p)
                for (p, h), (pr, inv, _) in zip(jobs, sm):
                    if n[0] == "s":
                        pbuf[h, :, pl.ds(0, 512 + 256 * h)] = pr
                        ibuf[h] = inv
                    else:
                        o = _dot_nt(pr, _blockdiag(site_kv(c, 1, b, g, p, h))) * inv
                        c_ref[at(p, h)] = o.astype(BF16)
            elif n[0] == "y":
                h = int(n[1])
                pr, inv, stats = _softmax(_scores(yq[h], kf[1, hrows(2, 1)].astype(BF16), _masks(h)[:2]))
                yc[h] = (_dot_nt(pr, _blockdiag(vf[1, hrows(2, 1)].astype(BF16))) * inv).astype(BF16)
                if h == 0:
                    yl_s[0] = jnp.concatenate([jnp.zeros((1, 128), F32), _pack(_lse(stats, 32), 4, 2)], axis=0)
                else:
                    yl_s[1] = _pack(_lse(stats, 128), 2, 0)
            elif n == "u":
                a = a1r.at[1, 0, 1]
                pr, inv, stats = _softmax(_scores(qa[pl.ds(384, 128), pl.ds(128, 128)], a[pl.ds(0, 128)],
                                                  _masks(1)[2:]))
                ubuf[...] = _dot_nt(pr, _blockdiag(a[pl.ds(128, 128)])) * inv
                yl_s[1] = _pack(_lse(stats, 128), 2, 0)
            elif n == "z":
                cx, _ = _merge([(ubuf[...], yl_s[1]), (yc[1].astype(F32), yl_r[1])], 2)
                ctxa[pl.ds(384, 128), pl.ds(128, 128)] = cx.astype(BF16)
            elif n[0] == "g":
                jobs = [(int(ch), b, p) for ch in n[1:] for b in range(2) for p in range(2)]
                lo = _iota((32, 128), 1) < 64
                ss = []
                for g, b, p in jobs:
                    q2 = qg[g, pl.ds(32 * b, 32), pl.ds(128 * p, 128)]
                    z = jnp.zeros_like(q2)
                    qs = jnp.concatenate([jnp.where(lo, q2, z), jnp.where(lo, z, q2)], axis=0)
                    ss.append(_dot(qs, kf[b, hrows(g, p)].astype(BF16)))
                ms = [jnp.max(x, axis=1, keepdims=True) for x in ss]
                es = [jnp.exp2(x - m) for x, m in zip(ss, ms)]
                ls = [jnp.sum(e, axis=1, keepdims=True) for e in es]
                outs = [_dot_nt(e.astype(BF16), vf[b, hrows(g, p)].astype(BF16))
                        for e, (g, b, p) in zip(es, jobs)]
                cols = {}
                for (g, b, p), o, m, l in zip(jobs, outs, ms, ls):
                    o = o * (1.0 / l)
                    gctx[g, pl.ds(32 * b, 32), pl.ds(128 * p, 128)] = jnp.where(lo, o[:32], o[32:])
                    lse = m + jnp.log2(l)
                    cols.setdefault((g, b), []).extend([lse[:32], lse[32:]])
                for (g, b), v in cols.items():
                    gl[g, pl.ds(b, 1)] = _pack(v, 4, 0)
            elif n[0] == "m":
                dst, srcs = n[1:].split(":")
                g = int(dst[2] if dst[0] == "C" else dst)
                ref = ctxa if g == c else ctxb
                terms = []
                for s in srcs.split(","):
                    if s == "g":
                        terms.append((gctx[g], gl[g]))
                    elif s == "s":
                        cx = jnp.concatenate([ref[pl.ds(0, 32)], ref[pl.ds(256, 32)]], axis=0)
                        terms.append((cx.astype(F32), l0[g] + yl_r[0] if c == 2 else l0[g]))
                    else:
                        terms.append((gr_c[gr_of[s]].astype(F32), gr_l[gr_of[s]]))
                cx, lse = _merge(terms, 4) if len(terms) > 1 else terms[0]
                if dst[0] == "C":
                    gs_c[gs_of[dst]] = cx.astype(BF16)
                    gs_l[gs_of[dst]] = lse
                else:
                    ref[pl.ds(0, 32)] = cx[:32].astype(BF16)
                    ref[pl.ds(256, 32)] = cx[32:].astype(BF16)
            elif n[0] in "pjk":
                blks = n[1:].split(",")
                cols = {"p": pl.ds(0, 256), "j": pl.ds(0, 128), "k": pl.ds(128, 128)}[n[0]]
                cx = jnp.concatenate([ctxa[prow(q), cols] for q in blks], axis=0)
                if c == 0:
                    cx = jnp.concatenate([cx, jnp.concatenate([ctxb[prow(q)] for q in blks], axis=0)], axis=1)
                    cols = pl.ds(0, 512)
                v = _dot(cx, wob[cols])
                for i, q in enumerate(blks):
                    o = orows(q)
                    o[...] = v[16 * i:16 * i + 16] + o[...] if n[0] == "k" else v[16 * i:16 * i + 16]
                    held[q + "L"] = held[q + "R"] = {str(c)}
            elif n[0] == "w":
                blks = n[1:].split(",")
                v = _dot(jnp.concatenate([ctxb[prow(q)] for q in blks], axis=0), wob[pl.ds(256, 256)])
                for i, q in enumerate(blks):
                    wbuf[prow(q)] = v[16 * i:16 * i + 16]
                    got |= {f"R{q}L_212", f"R{q}R_212"}
            else:
                piece, sites = n[1:4], n[4:]
                as_set = lambda t: set("012" if t == "F" else t)
                need, cols = as_set(sites), pl.ds(256 * "LR".index(piece[2]), 256)
                o = orows(piece).at[:, cols]
                cands = [(held[piece], lambda: o[...])] if piece in held else []
                for s, d, t in trees[piece]:
                    m = f"R{piece}_{s}{d}{t}"
                    if d == c and m in got:
                        cands.append((as_set(t), (lambda: wbuf[prow(piece), cols]) if as_ctx(s, d, t) else
                                      (lambda m=m: slot("r", m)[...].astype(F32))))
                acc, cov = None, set()
                for t, read in sorted(cands, key=lambda x: -len(x[0])):
                    if t <= need and not t & cov:
                        acc = read() if acc is None else acc + read()
                        cov |= t
                assert cov == need, (c, n)
                if held.get(piece, set()) < need:
                    o[...] = acc
                    held[piece] = need
                for s, d, t in trees[piece]:
                    m = f"R{piece}_{s}{d}{t}"
                    if (s, t) == (c, sites) and m in staged:
                        slot("s", m)[...] = acc.astype(BF16)

        def signal(sem, d):
            pl.semaphore_signal(sem, inc=1, device_id=(d,), device_id_type=MESH)

        def prologue(c):
            bar = pltpu.get_barrier_semaphore()
            lead = plan[c][:nlead[c]]
            if c == 0:
                signal(bar, 1)
                signal(bar, 3)
            elif c == 2:
                signal(bar, 0)
            else:
                pl.semaphore_wait(bar, 1)
                signal(rdy.at[c], 0)
                signal(bar, 2)
            for op in lead[:2]:
                load(c, op[2:]).start()
            if c == 2:
                pl.semaphore_wait(bar, 2)
                signal(rdy.at[2], 1)
                signal(rdy.at[2], 3)
            for op in lead[2:]:
                load(c, op[2:]).start()

        state = {c: ([{1, 2, 3}, {2}, set(), {2}][c], {}, set()) for c in range(4)}

        def program(c, stage):
            unseen, held, got = state[c]
            cut = plan[c].index("|")
            for op in plan[c][nlead[c]:cut] if stage == 0 else plan[c][cut + 1:]:
                kind, n = op[0], op[2:]
                if kind == "C":
                    compute(c, n, held, got)
                elif kind == "S":
                    d = message(n)[0]
                    if d in unseen:
                        pl.semaphore_wait(pltpu.get_barrier_semaphore() if c + d == 2 else rdy.at[d], 1)
                        unseen.discard(d)
                    for cp in copies(n):
                        cp.start()
                elif kind == "X":
                    for cp in copies(n, 0):
                        cp.wait_send()
                elif (c, n) in lsem_of:
                    load(c, n).wait()
                else:
                    for cp in copies(n, 1):
                        cp.wait_recv()
                    got.add(n)
            if stage == 1:
                for op in plan[c]:
                    if op[0] == "S" and "X" + op[1:] not in plan[c]:
                        for cp in copies(op[2:], 0):
                            cp.wait_send()
                assert not unseen and all(len(held[piece]) == 3 for piece in trees)

        for c in (1, 3, 2, 0):
            pl.when(me == c)(functools.partial(prologue, c))
        for stage, order in enumerate([(3, 2, 1, 0), (2, 3, 1, 0)]):
            for c in order:
                pl.when(me == c)(functools.partial(program, c, stage))

    vmem, dma = pltpu.VMEM, pltpu.SemaphoreType.DMA
    scratch = [
        vmem((2, 256, 512), F32), vmem((512, 256), F32), vmem((256, 512), F32),
        vmem((2, 1024, 256), F32), vmem((2, 1024, 256), F32),
        vmem((512, 256), BF16), vmem((512, 512), BF16),
        vmem((2, 2, 2, 2, 128, 256), BF16), vmem((2, 2, 2, 128, 256), BF16),
        vmem((2, 3, 2, 256, 128), BF16), vmem((2, 2, 2, 256, 128), BF16),
        vmem((512, 256), BF16), vmem((512, 256), BF16), vmem((4, 64, 256), BF16),
        vmem((4, 64, 256), F32), vmem((4, 2, 128), F32), vmem((4, 2, 128), F32),
        vmem((n_gs, 64, 256), BF16), vmem((n_gs, 2, 128), F32),
        vmem((n_gr, 64, 256), BF16), vmem((n_gr, 2, 128), F32),
        vmem((512, 256), BF16), vmem((512, 256), BF16),
        vmem((2, 128, 768), BF16), vmem((2, 128, 128), F32),
        vmem((2, 128, 128), BF16), vmem((2, 128, 128), BF16),
        vmem((2, 2, 128), F32), vmem((2, 2, 128), F32),
        vmem((128, 128), F32), vmem((512, 512), F32),
        vmem((n_sb, 16, 256), BF16), vmem((n_rb, 16, 256), BF16), vmem((2, 1, 128), F32),
        vmem((32, 256), BF16),
        dma((n_l,)), dma((n_s,)), dma((n_r,)), dma((n_s2,)), dma((n_r2,)),
        pltpu.SemaphoreType.REGULAR((4,)),
    ]
    return pl.pallas_call(
        body,
        out_shape=jax.ShapeDtypeStruct((2, 256, 512), F32),
        in_specs=[pl.BlockSpec(memory_space=pltpu.HBM)] * 5,
        out_specs=pl.BlockSpec(memory_space=pltpu.VMEM),
        scratch_shapes=scratch,
        compiler_params=pltpu.CompilerParams(
            collective_id=0, vmem_limit_bytes=40 * 1024 * 1024,
            disable_semaphore_checks=True),
        **debug,
    )


_PLAN = {
    0: """
        L:k041 L:xg L:wq L:k022 L:k051 L:v024 L:xr0 L:k002 L:v002 L:k124 L:v124 L:k062 L:v062 L:xr1
        L:k102 L:v102 L:wo0g L:k162 L:v162 W:k041 C:ck020 W:wq C:cq W:xg C:qg W:k022 C:ck010 C:ck011
        W:k051 C:ck021 S:K010 S:Qg001 S:K020p0 S:K020p1 S:Qg003 W:v024 C:cv010 S:V010 S:K011 C:cv020
        C:cv011 S:V011 C:cv021 S:K020r S:V020 S:K021 S:V021 W:xr0 C:q002 W:k002 W:v002 W:A000a
        W:A000b X:K020p0 X:K020p1 X:Qg003 W:A000v C:a00_00_01 W:k124 C:ck120 C:ck110 W:v124 C:cv110
        S:K110 C:ck111 C:cv120 S:K120 W:xr1 C:q102 W:wo0g C:cw0g W:A001 C:a00_10_11 S:V110 S:V120
        C:cv111 S:K111 W:Q300 W:k062 W:v062 C:a03_00_10 W:k102 W:v102 X:K010 X:Qg001 X:V010 X:K011
        X:V011 X:K020r X:V020 X:K021 X:V021 W:A100 C:a10_00_01 W:Y100 C:y0 S:V111 S:Z00a W:Y301 C:y1
        S:Z00b W:W3001 W:W3013 W:W3043 W:W3079 C:p02,03,04,05,06,07 S:Z01a C:f02L0 C:f07R0 S:T03
        S:Z01b C:f07L0 C:f02R0 C:f05L0 S:R07R_030 C:f05R0 X:K110 X:K120 W:Q301 W:A030 W:A031
        C:a03_01_11 S:R05R_030 S:R07L_030 C:p08,09,0a,0b,0c,0d,0e,0f C:f0aL0 S:R02L_010 C:f08L0
        C:f06L0 S:R02R_010 C:f09L0 C:f0bL0 C:f0fR0 C:f0cL0 C:f09R0 C:f06R0 S:R0bL_010 S:R0aL_030
        S:R09L_010 S:R05L_030 C:f0dL0 C:f0fL0 C:f0aR0 C:f0eR0 C:f08R0 C:f0cR0 S:R08R_010 S:R0dL_030
        C:f0eL0 S:R0cL_030 C:f0dR0 W:A101 C:a10_10_11 S:R0aR_030 C:f0bR0 S:R0cR_030 S:R0eR_030
        S:R09R_010 S:R0eL_030 S:R0dR_030 S:R0fL_030 S:R0fR_030 W:Q311 W:k162 W:v162 W:A130 C:a13_01
        S:R06L_030 S:R06R_030 S:R08L_010 S:R0bR_010 X:V110 X:V120 X:K111 X:Z00a X:Z00b X:Z01a X:T03
        X:Z01b X:R07R_030 X:R05R_030 X:R07L_030 X:R0aL_030 X:R05L_030 W:A131 C:a13_11 W:R03L_1012
        C:f03LF S:R03L_03F S:R03L_01F W:R03R_1012 C:f03RF S:R03R_01F C:p18,19,1a,1b,1c,1d,1e,1f
        C:f1aR0 S:R1aR_010 C:f18L0 C:f19L0 C:f19R0 C:f1eL0 S:R1eL_030 C:f1dR0 S:R19R_010 W:R09R_1012
        C:f09RF C:f1dL0 C:f1eR0 C:f1cL0 C:f1aL0 S:R1dL_030 S:R03R_03F C:f18R0 C:f1fR0 S:R1dR_030
        W:R0bL_1012 C:f0bLF C:f1bL0 S:R18L_010 S:R19L_010 S:R18R_010 C:f1bR0 C:f1fL0 S:R1eR_030
        C:f1cR0 S:R1fL_030 S:R1fR_030 W:Q310 C:a13_00_10 S:R1bL_010 S:R1aL_010 C:p12,13,14,15,16,17
        W:R13R_1012 C:f13RF C:f15R0 S:R15R_010 C:f17R0 W:R04R_1012 C:f04RF S:R17R_030 S:R1bR_010
        S:R1cL_010 W:Cg0_30 C:m0:s,Cg0_30 S:R1cR_030 S:R13R_01F W:R12L_1012 C:f12LF W:Cg3_30
        C:m3:s,Cg3_30 W:R13L_1012 C:f13LF S:R12L_03F W:R14L_1012 C:f14LF S:R14L_03F S:R12L_01F
        C:p00,01,10,11 W:R14R_1012 C:f14RF S:R14R_03F C:f10R0 W:R0cR_3012 C:f0cRF C:f10L0 S:R10L_010
        C:f01L0 S:R10R_010 W:R16L_1012 C:f16LF W:R0cL_3012 C:f0cLF W:R05L_30F C:f05LF S:R16L_03F
        X:V111 X:R02L_010 X:R02R_010 X:R0bL_010 X:R09L_010 X:R08R_010 X:R0dL_030 X:R0cL_030
        X:R0aR_030 X:R0cR_030 X:R0eR_030 X:R09R_010 X:R0eL_030 X:R0dR_030 X:R0fL_030 X:R0fR_030
        X:R06L_030 X:R06R_030 X:R08L_010 X:R0bR_010 X:R03L_03F X:R03L_01F X:R03R_01F X:R1aR_010
        X:R1eL_030 X:R19R_010 X:R1dL_030 X:R03R_03F X:R1dR_030 X:R18L_010 X:R19L_010 X:R18R_010
        X:R1eR_030 X:R1fL_030 X:R1fR_030 X:R1bL_010 X:R1aL_010 W:R15L_1012 C:f15LF W:R05R_30F
        C:f05RF S:R13L_03F C:f11R0 W:R0aL_3012 C:f0aLF X:R15R_010 X:R17R_030 W:R17L_1012 C:f17LF
        W:R04L_1012 C:f04LF S:R11R_010 S:R15L_03F C:f11L0 X:R1bR_010 X:R1cR_030 W:R16R_1012 C:f16RF
        W:R08R_1012 C:f08RF S:R16R_03F W:R0eL_3012 C:f0eLF S:R01L_010 S:R04R_01F W:R12R_1012 C:f12RF
        W:R0dL_3012 C:f0dLF C:f01R0 S:R11L_010 W:R09L_1012 C:f09LF S:R01R_010 S:R17L_03F S:R09L_03F
        W:R0fR_3012 C:f0fRF W:R07L_30F C:f07LF S:R13R_03F W:R0eR_3012 C:f0eRF X:R1cL_010 X:R13R_01F
        X:R12L_03F X:R14L_03F W:R19R_10F C:f19RF S:R12R_03F W:R0bR_1012 C:f0bRF S:R13L_01F
        W:R1bR_1012 C:f1bRF S:R12R_01F S:R04R_03F | X:R12L_01F X:R14R_03F X:R10L_010 X:R16L_03F
        W:R19L_10F C:f19LF W:R0dR_3012 C:f0dRF W:R18L_10F C:f18LF W:R06R_30F C:f06RF X:R10R_010
        X:R13L_03F W:R1bL_10F S:R1bL_03F S:R06R_01F W:R07R_30F C:f07RF X:R11R_010 X:R15L_03F
        W:R02R_30F C:f02RF W:R02L_30F C:f02LF S:R04L_01F W:R0fL_3012 C:f0fLF S:R04L_03F C:f1bLF
        W:R18R_10F C:f18RF W:R08L_1012 C:f08LF X:R16R_03F X:R01L_010 X:R04R_01F X:R17L_03F
        W:R15R_10F C:f15RF S:R15R_03F W:R17R_30F S:R17R_01F X:R11L_010 X:R09L_03F W:R00L_1012
        C:f00LF S:R00L_01F S:R00L_03F W:R1cR_30F C:f1cRF W:R1dL_30F C:f1dLF W:R00R_1012 C:f00RF
        W:R0aR_3012 C:f0aRF S:R00R_03F S:R1cR_01F W:R06L_30F C:f06LF X:R01R_010 X:R13R_03F
        X:R12R_03F X:R13L_01F W:R11L_1012 C:f11LF S:R00R_01F S:R11L_03F W:R1dR_30F C:f1dRF
        X:R12R_01F X:R04R_03F W:R01L_1012 C:f01LF C:f17RF S:R01L_03F W:R1fL_30F S:R1fL_01F
        W:R1aL_10F C:f1aLF C:f1fLF X:R1bL_03F X:R06R_01F W:R01R_1012 C:f01RF W:R1fR_30F C:f1fRF
        S:R01R_03F S:R1dR_01F X:R04L_01F X:R04L_03F W:R11R_1012 C:f11RF W:R1eR_30F S:R1eR_01F
        S:R11R_03F C:f1eRF X:R15R_03F X:R17R_01F W:R10L_1012 C:f10LF W:R1aR_30F C:f1aRF X:R00L_01F
        X:R00L_03F W:R1cL_10F C:f1cLF W:R1eL_30F C:f1eLF X:R00R_03F X:R1cR_01F W:R10R_1012 C:f10RF
    """.split(),
    1: """
        L:k001a L:k001b L:v001l L:k011l L:v011l L:xg L:wq L:k044l L:v044l L:k002h L:v002h L:k062h
        L:v062h L:k102 L:v102 L:k162 L:v162 L:k142l L:v142l L:xr0 L:k022 L:v022 L:k142h L:v142h
        L:k042h L:v042h L:wo0g L:xr1 L:k122 L:v122 W:k001a C:ca000a S:A000a W:k001b C:ca000b S:A000b
        W:v001l C:ca000v S:A000v W:k011l W:v011l C:ca001 S:A001 W:wq C:cq W:xg C:qg S:Qg112 W:k044l
        W:v044l C:ca020 S:A020 C:ca030 S:A030 C:ca031 S:A031 C:ca021 W:k102 W:v102 C:ca100 S:A100
        C:ca101 W:Qg001 S:Qg012 S:A021 W:k162 W:v162 C:ca130 C:ca131 W:k142l W:v142l C:ca120 S:A120
        C:ca121 W:xr0 C:q002 W:Qg321 W:k002h W:v002h W:k062h W:v062h C:g03 W:K010 W:V010 W:k022
        W:v022 C:a01_00_01 W:Y210 S:Y100 C:mCg0_12:g S:Cg0_12 C:mCg3_12:g S:A101 S:A130 S:Cg3_12
        W:wo0g C:cw0g W:K011 X:A000a X:A000b X:A000v X:A001 X:Qg112 X:A020 X:A030 X:A031 X:Qg012
        X:A021 W:V011 C:a01_10_11 S:A121 C:p08,09,0a,0b,0c,0d,0e,0f C:f0aR1 C:f0cR1 C:f0cL1 C:f0fR1
        C:p02,03,04,05,06,07 S:R0aR_121 C:f07L1 C:f0dR1 S:R0cL_121 C:f05R1 W:xr1 C:q102 C:f0dL1
        W:Qg221 W:k042h W:v042h W:k142h W:v142h W:k122 W:v122 C:g21 S:R05R_121 S:R07L_121 S:R0dL_121
        C:f0eR1 C:f06L1 S:A131 C:f0aL1 S:R0cR_121 S:R0eR_121 S:R0aL_121 W:K110 X:A100 X:A120 X:Y100
        X:Cg0_12 X:A101 X:Cg3_12 W:V110 C:a11_00_01 C:f0eL1 C:f0fL1 C:f05L1 S:R0fL_121 S:R05L_121
        W:H0b W:W2104 W:W2144 W:W2188 C:w0b C:f06R1 C:j18,19,1a,1b,1c,1d,1e,1f W:H03 W:H08 C:w03,08
        S:R0eL_121 W:H02 W:H04 W:H09 C:w02,04,09 C:f04L12 C:f07R1 C:f04R12 S:R07R_121 C:f09R12
        C:f03R12 C:f08R12 C:f0bL12 S:R0dR_121 S:R06L_121 C:f09L12 C:f03L12 C:f08L12 S:R03R_1012
        S:R03L_1012 S:R0fR_121 S:R0bL_1012 S:R09R_1012 S:R04R_1012 C:f0bR12 S:R04L_1012 S:R06R_121
        S:R08R_1012 W:K111 C:s11_10_11 C:j12,13,14,15,16,17 S:R09L_1012 S:R0bR_1012 S:R08L_1012
        W:H13 C:w13 W:H12 C:w12 X:A130 X:A121 X:R0aR_121 X:R0cL_121 X:R05R_121 X:R07L_121 X:R0dL_121
        X:A131 X:R0cR_121 X:R0eR_121 X:R0aL_121 X:R0fL_121 X:R05L_121 X:R0eL_121 X:R07R_121
        X:R0dR_121 X:R03R_1012 X:R03L_1012 W:V111 C:o11_10 W:R02L_010 C:f02LF S:R02L_12F
        C:k12,13,14,15,16,17 C:f13L12 C:f12L12 C:f13R12 C:f12R12 W:R02R_010 C:f02RF C:f17R1
        S:R17R_121 S:R13R_1012 S:R12L_1012 S:R02R_12F C:o11_11 S:R12R_1012
        C:k18,19,1a,1b,1c,1d,1e,1f C:f1dL1 S:R13L_1012 S:R1dL_121 W:H14 W:H15 C:w14,15 C:f14L12
        S:R14L_1012 C:f1cR1 C:f1fL1 S:R1cR_121 C:f14R12 S:R14R_1012 C:f1dR1 C:f1fR1 C:f1eR1
        W:R08R_010 C:f08RF S:R1dR_121 W:H16 W:H1a C:w16,1a C:f16L12 W:R0bL_010 C:f0bLF S:R16L_1012
        C:f15L12 C:f1eL1 S:R15L_1012 S:R1fL_121 S:R1fR_121 W:H17 W:H1b C:w17,1b W:R0bR_010 C:f0bRF
        C:f17L12 S:R17L_1012 S:R1eR_121 W:R03R_01F C:f03RF C:f16R12 S:R16R_1012 C:f1bR12 W:H18 W:H19
        C:w18,19 W:R1aR_010 C:f1aR01 S:R1aR_1201 S:R1eL_121 S:R1bR_1012 X:R06L_121 X:R0fR_121
        X:R0bL_1012 X:R09R_1012 X:R04R_1012 X:R04L_1012 X:R06R_121 X:R08R_1012 X:R09L_1012
        X:R0bR_1012 X:R08L_1012 X:R02L_12F X:R17R_121 X:R13R_1012 X:R12L_1012 X:R02R_12F X:R12R_1012
        X:R13L_1012 X:R1dL_121 W:R19R_010 C:f19R01 W:R09R_010 C:f09RF S:R08R_12F C:f19RF S:R19R_10F
        S:R0bR_12F W:H1c C:w1c W:R18L_010 C:f18L01 C:f18LF S:R18L_10F S:R09R_12F X:R14L_1012
        X:R1cR_121 X:R14R_1012 W:R19L_010 C:f19L01 C:f19LF S:R19L_10F S:R0bL_12F W:Cg1_21
        C:m1:s,g,Cg1_21 W:R1bL_010 C:f1bLF S:R1bL_10F S:R19R_1201 W:R18R_010 C:f18R01 S:R18R_1201
        C:f18RF S:R18R_10F S:R18L_1201 S:R19L_1201 C:p00,01 W:R08L_010 C:f08LF W:R1aL_010 C:f1aL01
        C:f1aLF W:R03L_01F C:f03LF S:R1aL_10F W:Cg2_21 C:m2:g,Cg2_21 W:R15R_010 C:f15RF S:R15R_10F
        C:w00,11 C:f00L12 S:R00L_1012 C:p10,11 W:R1cL_010 C:f1cL01 C:f11L12 C:f00R12 W:R0cL_21F
        C:f0cLF S:R1aL_1201 C:f1cLF S:R00R_1012 C:w01,10 W:R07L_21F C:f07LF S:R11L_1012 C:f01L12
        S:R08L_12F W:R12L_01F C:f12LF S:R1cL_1201 W:R1bR_010 C:f1bRF C:f10L12 S:R01L_1012 C:f11R12
        X:R1dR_121 X:R16L_1012 X:R15L_1012 X:R1fL_121 X:R1fR_121 X:R17L_1012 X:R1eR_121 X:R16R_1012
        X:R1aR_1201 X:R1eL_121 X:R1bR_1012 X:R08R_12F X:R19R_10F X:R0bR_12F X:R18L_10F X:R09R_12F
        X:R19L_10F X:R1bL_10F W:R10L_010 C:f10LF C:f01R12 W:R13R_01F C:f13RF C:f10R12 S:R01R_1012
        S:R11R_1012 S:R10L_1012 X:R0bL_12F X:R18R_10F W:R10R_010 C:f10RF S:R10L_12F W:R05R_21F
        C:f05RF S:R10R_12F X:R19R_1201 X:R1aL_10F W:R11R_010 C:f11RF S:R1cL_10F W:R0dL_21F C:f0dLF
        S:R1bR_12F W:R0aL_21F C:f0aLF S:R11R_12F S:R10R_1012 S:R15R_12F S:R03R_12F W:R0eL_21F
        C:f0eLF C:f1aRF W:R09L_010 C:f09LF | X:R18R_1201 X:R18L_1201 X:R19L_1201 X:R15R_10F
        X:R00L_1012 W:R05L_21F C:f05LF X:R1aL_1201 X:R00R_1012 W:R0fR_21F C:f0fRF W:R04R_01F
        S:R04R_12F W:R11L_010 C:f11LF W:R01L_010 C:f01LF X:R11L_1012 W:R01R_010 C:f01RF S:R09L_12F
        S:R03L_12F C:f04RF X:R08L_12F X:R01L_1012 W:R13L_01F C:f13LF X:R1cL_1201 X:R01R_1012
        W:R12R_01F C:f12RF S:R11L_12F W:R1dL_21F C:f1dLF W:R0cR_21F C:f0cRF W:R0eR_21F C:f0eRF
        S:R01L_12F S:R01R_12F X:R11R_1012 X:R10L_1012 X:R10L_12F X:R10R_12F W:R04L_01F C:f04LF
        W:R06R_01F C:f06RF W:R0dR_21F C:f0dRF W:R1fR_21F C:f1fRF W:R1eL_21F C:f1eLF X:R1cL_10F
        X:R1bR_12F X:R11R_12F W:R0fL_21F C:f0fLF X:R10R_1012 W:R00L_01F C:f00LF W:R17R_01F C:f17RF
        W:R0aR_21F C:f0aRF X:R15R_12F X:R03R_12F W:R14L_21F C:f14LF W:R07R_21F C:f07RF S:R04L_12F
        W:R00R_01F C:f00RF W:R06L_21F C:f06LF W:R1cR_01F C:f1cRF X:R04R_12F W:R1fL_01F C:f1fLF
        W:R14R_21F C:f14RF W:R16L_21F C:f16LF X:R09L_12F W:R1dR_01F C:f1dRF W:R15L_21F C:f15LF
        X:R03L_12F X:R11L_12F W:R16R_21F C:f16RF W:R1eR_01F C:f1eRF X:R01L_12F W:R17L_21F C:f17LF
    """.split(),
    2: """
        L:xg L:wq L:wo04 L:xr0 L:xr1 L:wo44 L:wo88 L:k202 L:v202 L:k262 L:v262 L:k222 L:v222 L:k242
        L:v242 W:wq C:cq W:xg C:qg S:Qg221 S:Qg223 W:wo04 C:cw04 S:W2104 W:xr0 C:q002 W:Qg332a
        W:Qg332b S:Qg321 W:xr1 C:q102 S:Y210 W:Qg112 S:Qg123 S:Y231 W:wo44 C:cw44 S:W2144 W:wo88
        C:cw88 S:W2188 X:Qg221 X:Qg223 W:K020r W:K020f0 W:K020f1 X:W2104 X:Qg321 X:Qg123 W:V020
        W:A020 C:a02_00_01 W:Qg012 W:k202 W:v202 W:k262 W:v262 C:g03 W:k222 W:v222 C:g1 W:K021
        X:Y210 X:Y231 X:W2144 W:V021 W:A021 C:a02_10_11 W:Cg0_12 C:mCg0_23:g,Cg0_12 S:H08 S:H04
        S:Cg0_23 C:p05,06,07 S:H0b W:Cg3_12 C:mCg3_23:g,Cg3_12 S:H09 S:Cg3_23 S:H03 S:H02
        C:p0a,0c,0d,0e,0f W:K120 W:A120 C:s12_00_01 W:k242 W:v242 C:g2 W:R0aR_121 C:f0aR12 W:V120
        C:o12_00 W:R0cL_121 C:f0cL12 W:R05R_121 C:f05R12 S:R0cL_2312 S:R0aR_2312 W:Z00a S:H13 S:H12
        W:A121 C:u W:R07L_121 C:f07L12 W:R0dL_121 C:f0dL12 S:R0dL_2312 W:Z00b S:H17 S:R05R_2312
        C:o12_01 W:R0eR_121 C:f0eR12 W:R0aL_121 C:f0aL12 S:R07L_2312 S:H15 S:R0aL_2312 S:H14
        W:R0cR_121 C:f0cR12 S:R0cR_2312 S:H16 W:Z01a X:W2188 X:H08 X:H04 X:Cg0_23 X:H0b X:H09
        X:Cg3_23 X:H03 X:H02 X:R0cL_2312 X:H13 W:Z01b C:z S:H1b W:R05L_121 C:f05L12 S:R05L_2312
        S:H1a W:R0eL_121 C:f0eL12 S:H18 W:R0fL_121 C:f0fL12 S:H1c S:H19 S:R0eL_2312 S:R0fL_2312
        X:R0aR_2312 X:H12 X:R0dL_2312 X:H17 X:R05R_2312 W:R0dR_121 C:f0dR12 S:R0eR_2312 C:p17
        S:R0dR_2312 W:R06L_121 C:f06L12 W:Cg1_32 C:mCg1_21:g,Cg1_32 X:R07L_2312 X:H15 X:R0aL_2312
        X:H14 W:R06R_121 C:f06R12 W:R0fR_121 C:f0fR12 S:R0fR_2312 S:R06R_2312 S:Cg1_21
        C:p18,19,1a,1c,1d,1e,1f W:R07R_121 C:f07R12 S:R07R_2312 W:Cg2_32 C:mCg2_21:s,g,Cg2_32
        S:R06L_2312 S:Cg2_21 X:R0cR_2312 X:H16 X:H1b X:R05L_2312 X:H1a X:H18 X:H1c X:H19 X:R0eL_2312
        X:R0fL_2312 X:R0eR_2312 X:R0dR_2312 W:R02L_12F S:R02L_23F | X:R0fR_2312 X:R06R_2312
        W:R02R_12F C:f02RF W:R17R_121 C:f17R12 W:R07L_32F S:R07L_21F S:R02R_23F W:R05R_32F
        S:R05R_21F S:R17R_2312 W:R0cL_32F S:R0cL_21F W:R0cR_32F S:R0cR_21F X:Cg1_21 X:R07R_2312
        X:R06L_2312 W:R1dL_121 C:f1dL12 W:R0aR_32F S:R0aR_21F S:R1dL_2312 W:R0dL_32F S:R0dL_21F
        W:R1cR_121 C:f1cR12 S:R1cR_2312 X:R02L_23F W:R1dR_121 C:f1dR12 S:R1dR_2312 W:R0eL_32F
        S:R0eL_21F W:R1fL_121 C:f1fL12 S:R1fL_2312 C:f02LF X:Cg2_21 W:R1fR_121 C:f1fR12 W:R0aL_32F
        S:R0aL_21F C:f0cRF S:R1fR_2312 X:R07L_21F X:R02R_23F W:R1eR_121 C:f1eR12 S:R1eR_2312
        X:R05R_21F X:R17R_2312 W:R1aR_1201 C:f1aRF S:R1aR_23F W:R06R_320 C:f06RF W:R0eR_32F
        S:R0eR_21F W:R05L_32F S:R05L_21F X:R0cL_21F X:R1dL_2312 W:R1eL_121 C:f1eL12 S:R1eL_2312
        X:R0cR_21F X:R1cR_2312 W:R08R_12F S:R08R_23F C:f07LF W:R0fR_32F S:R0fR_21F X:R0aR_21F
        X:R1dR_2312 X:R1fL_2312 W:R0dR_32F S:R0dR_21F C:f05LF W:R1dL_320 C:f1dLF W:R09R_12F
        S:R09R_23F S:R1dL_21F W:R1eL_320 C:f1eLF W:R0bR_12F S:R0bR_23F W:R07R_32F S:R07R_21F C:f05RF
        X:R0dL_21F X:R0eL_21F X:R0aL_21F X:R1fR_2312 X:R1eR_2312 W:R19R_1201 C:f19RF S:R1eL_21F
        W:R0bL_12F S:R0bL_23F X:R1aR_23F X:R0eR_21F W:R18R_1201 C:f18RF W:R1fR_320 C:f1fRF C:f0bLF
        S:R19R_23F S:R1fR_21F X:R05L_21F X:R1eL_2312 W:R18L_1201 C:f18LF W:R0fL_32F S:R0fL_21F
        C:f0cLF S:R18R_23F C:f09RF C:f0bRF S:R18L_23F W:R06L_32F S:R06L_21F C:f0eRF X:R08R_23F
        X:R0fR_21F X:R0dR_21F W:R1aL_1201 C:f1aLF C:f07RF W:R19L_1201 C:f19LF S:R1aL_23F W:R14L_32F
        C:f14LF S:R19L_23F S:R14L_21F W:R14R_32F S:R14R_21F W:R08L_12F C:f08LF S:R08L_23F C:f0dLF
        C:f14RF C:f0fRF C:f0aRF X:R09R_23F X:R1dL_21F X:R0bR_23F X:R07R_21F W:R1cL_1201 C:f1cLF
        C:f06LF C:f0eLF C:f0aLF W:R16L_32F S:R16L_21F W:R10L_12F S:R10L_23F C:f10LF W:R12L_32F
        C:f12LF W:R1fL_32F C:f1fLF S:R1cL_23F W:R17R_320 C:f17RF W:R15L_32F S:R15L_21F C:f0dRF
        W:R10R_12F S:R10R_23F C:f0fLF C:f15LF C:f16LF C:f10RF W:R16R_32F S:R16R_21F C:f16RF
        X:R1eL_21F X:R0bL_23F X:R19R_23F X:R1fR_21F X:R0fL_21F X:R18R_23F X:R18L_23F W:R17L_32F
        S:R17L_21F W:R11R_12F C:f11RF W:R1bR_12F C:f1bRF C:f17LF S:R1bR_23F X:R06L_21F X:R1aL_23F
        X:R19L_23F X:R14L_21F W:R1dR_32F C:f1dRF C:f08RF X:R14R_21F X:R08L_23F W:R13L_32F C:f13LF
        W:R1eR_32F C:f1eRF W:R04R_12F C:f04RF W:R15R_12F C:f15RF X:R16L_21F X:R10L_23F X:R15L_21F
        W:R09L_12F C:f09LF W:R12R_32F C:f12RF X:R1cL_23F X:R16R_21F W:R03L_12F C:f03LF X:R10R_23F
        X:R17L_21F W:R11L_12F C:f11LF W:R13R_32F C:f13RF W:R1bL_32F C:f1bLF W:R03R_12F C:f03RF
        X:R1bR_23F W:R01L_12F C:f01LF W:R1cR_32F C:f1cRF W:R00L_32F C:f00LF W:R01R_12F C:f01RF
        W:R04L_12F C:f04LF W:R00R_32F C:f00RF
    """.split(),
    3: """
        L:wo01 L:wo13 L:xg L:wqa L:wqb L:wo43 L:xr0 L:wo79 L:xr1 L:k202 L:v202 L:k262 L:v262 L:k224
        L:v224 W:wo01 C:cw01 S:W3001 W:wo13 C:cw13 S:W3013 W:wqa C:cqa W:xg C:qga S:Qg332a W:wqb
        C:cqb C:qgb S:Qg332b W:wo43 C:cw43 S:W3043 X:W3001 W:K020p0 S:K020f0 W:K020p1 S:K020f1 W:xr0
        C:q001 S:Q300 C:q011 W:wo79 C:cw79 S:W3079 W:xr1 C:q102 W:Qg003 W:k202 W:v202 W:k262 W:v262
        C:g03 W:Y231 S:Y301 S:Q301 S:Q311 W:Qg123 W:Qg223 W:k224 W:v224 C:g12 C:mCg1_32:g
        C:mCg2_32:g S:Q310 | X:W3013 X:Qg332a X:Qg332b X:W3043 X:K020f0 X:K020f1 X:Q300 X:W3079
        X:Y301 X:Q301 W:Cg0_23 C:mCg0_30:g,Cg0_23 X:Q311 W:T03 S:Cg1_32 W:Cg3_23 C:mCg3_30:g,Cg3_23
        S:Cg3_30 S:Cg2_32 S:Cg0_30 X:Q310 W:R0dL_2312 W:R0dL_030 C:f0dLF W:R0cL_2312 W:R0cL_030
        C:f0cLF S:R0dL_32F W:R05R_2312 W:R05R_030 C:f05RF S:R0cL_32F S:R0dL_3012 S:R05R_30F X:Cg1_32
        X:Cg3_30 W:R07L_2312 W:R07L_030 C:f07LF W:R0aR_2312 S:R0aR_3012 S:R05R_32F S:R07L_32F
        W:R0cR_2312 W:R0cR_030 C:f0cRF S:R07L_30F S:R0cR_32F W:R0aR_030 C:f0aRF W:R0aL_2312
        W:R0aL_030 C:f0aLF X:Cg2_32 W:R05L_2312 W:R05L_030 C:f05LF S:R0aR_32F S:R0aL_3012 S:R05L_30F
        S:R05L_32F S:R0aL_32F W:R0eL_2312 W:R0eL_030 C:f0eLF S:R0cL_3012 S:R0eL_32F S:R0cR_3012
        S:R0eL_3012 X:Cg0_30 X:R0dL_32F X:R0cL_32F X:R0dL_3012 X:R05R_30F X:R0aR_3012 X:R05R_32F
        W:R06R_030 S:R06R_320 W:R0fL_2312 S:R0fL_3012 W:R0eR_2312 W:R0eR_030 C:f0eRF W:R0fR_2312
        S:R0fR_3012 W:R0dR_2312 S:R0dR_3012 W:R0fL_030 C:f0fLF S:R0fL_32F X:R07L_32F X:R07L_30F
        X:R0cR_32F W:R06R_2312 C:f06RF S:R0eR_32F S:R0eR_3012 W:R0dR_030 C:f0dRF W:R0fR_030 C:f0fRF
        S:R06R_30F S:R0fR_32F X:R0aR_32F X:R0aL_3012 W:R07R_2312 W:R07R_030 C:f07RF S:R07R_32F
        X:R05L_30F X:R05L_32F X:R0aL_32F X:R0cL_3012 W:R06L_2312 W:R06L_030 C:f06LF S:R06L_30F
        W:R1dL_030 S:R1dL_320 S:R07R_30F S:R0dR_32F W:R1eL_030 S:R1eL_320 X:R0eL_32F X:R0cR_3012
        X:R0eL_3012 W:R02L_23F S:R02L_30F S:R06L_32F X:R06R_320 X:R0fL_3012 X:R0fR_3012 X:R0fL_32F
        W:R1fR_030 S:R1fR_320 W:R02R_23F C:f02RF S:R02R_30F X:R0dR_3012 X:R0eR_32F X:R0fR_32F
        W:R17R_2312 W:R17R_030 C:f17RF S:R17R_320 S:R17R_30F X:R0eR_3012 X:R07R_32F W:R1dL_2312
        C:f1dLF W:R12L_03F S:R12L_32F S:R1dL_30F W:R1cR_2312 W:R1cR_030 C:f1cRF C:f12LF S:R1cR_30F
        W:R14L_03F S:R14L_32F W:R03R_03F C:f03RF W:R1dR_2312 W:R1dR_030 C:f1dRF W:R14R_03F
        S:R14R_32F S:R1dR_30F W:R1fL_2312 W:R1fL_030 C:f1fLF C:f02LF S:R1fL_32F S:R1fL_30F
        X:R06R_30F X:R06L_30F X:R1dL_320 X:R07R_30F X:R0dR_32F X:R1eL_320 X:R02L_30F X:R06L_32F
        W:R1fR_2312 C:f1fRF C:f14RF S:R1fR_30F W:R16L_03F S:R16L_32F X:R1fR_320 X:R02R_30F
        W:R1eR_2312 W:R1eR_030 C:f1eRF W:R15L_03F S:R15L_32F S:R1eR_30F X:R17R_320 X:R17R_30F
        X:R12L_32F X:R1dL_30F W:R16R_03F C:f16RF S:R16R_32F W:R1aR_23F S:R1aR_30F C:f1aRF
        W:R1eL_2312 C:f1eLF W:R17L_03F S:R17L_32F S:R1eL_30F W:R08R_23F C:f08RF W:R13L_03F C:f13LF
        W:R09L_03F C:f09LF S:R1eR_32F S:R1dR_32F C:f14LF S:R13L_32F C:f15LF C:f16LF X:R1cR_30F
        X:R14L_32F X:R14R_32F X:R1dR_30F X:R1fL_32F X:R1fL_30F W:R12R_03F C:f12RF W:R0bR_23F C:f0bRF
        W:R09R_23F C:f09RF W:R03L_03F C:f03LF C:f17LF S:R12R_32F W:R13R_03F S:R13R_32F X:R1fR_30F
        X:R16L_32F X:R15L_32F X:R1eR_30F W:R0bL_23F C:f0bLF W:R1bL_03F C:f1bLF S:R1bL_32F C:f13RF
        W:R04R_03F C:f04RF S:R1cR_32F W:R19R_23F C:f19RF W:R04L_03F C:f04LF X:R16R_32F X:R1aR_30F
        X:R17L_32F X:R1eL_30F W:R15R_03F C:f15RF X:R1eR_32F W:R00L_03F S:R00L_32F C:f00LF W:R18R_23F
        C:f18RF W:R18L_23F C:f18LF X:R1dR_32F W:R00R_03F S:R00R_32F C:f00RF W:R19L_23F C:f19LF
        W:R1aL_23F C:f1aLF X:R13L_32F X:R12R_32F W:R08L_23F C:f08LF W:R01L_03F C:f01LF W:R11L_03F
        C:f11LF W:R10L_23F C:f10LF X:R13R_32F X:R1bL_32F W:R1cL_23F C:f1cLF W:R11R_03F C:f11RF
        W:R01R_03F C:f01RF W:R10R_23F C:f10RF X:R1cR_32F X:R00L_32F W:R1bR_23F C:f1bRF
    """.split(),
}

_TREES = {
    "010 1201 212 10F 23F": "18L 18R 19L 19R 1aL 1cL",
    "010 1201 212 23F 30F": "1aR",
    "030 121 2312 30F 01F 32F": "1cR 1dR 1eR 1fL",
    "030 121 2312 30F 32F 21F": "05L 05R 06L 07L 07R",
    "121 030 2312 320 21F 30F": "1dL 1eL 1fR",
    "121 030 2312 320 30F 01F": "06R 17R",
    "121 2312 3012 030 32F 21F": "0aL 0aR 0cL 0cR 0dL 0dR 0eL 0eR 0fL 0fR",
    "212 010 1012 03F 12F": "01L 01R 09L 11L 11R",
    "212 010 1012 12F 23F": "08L 08R 09R 0bL 0bR 10L 10R 1bR",
    "212 010 10F 03F 32F": "1bL",
    "212 010 12F 10F 03F": "15R",
    "212 010 12F 23F 30F": "02L 02R",
    "212 1012 01F 03F 32F": "00L 00R 12L 12R 13L 13R",
    "212 1012 03F 01F 12F": "03L 03R 04L 04R",
    "212 1012 03F 32F 21F": "14L 14R 15L 16L 16R 17L",
}
_AR = {piece: [(int(w[0]), int(w[1]), w[2:]) for w in steps.split()]
       for steps, pieces in _TREES.items() for piece in pieces.split()}


def pallas_dist_sparse_attn_localglobal_htp_kvseq_b2_sq256_skv256_hq4_dh64_kernel(
    x: jax.Array,
    Wq: jax.Array,
    K_ext: jax.Array,
    V_ext: jax.Array,
    Wo: jax.Array,
):
    kt = jnp.transpose(K_ext, (0, 2, 3, 1)).reshape(2, 1024, 256)
    vt = jnp.transpose(V_ext, (0, 2, 3, 1)).reshape(2, 1024, 256)
    return _build(_PLAN, _AR)(x, Wq, kt, vt, Wo)
```
